```python
import numpy as np

kernel_name = "dist_moe_shared_ep_outshard_n512_d256_e2_h512"

def setup_inputs():
    x = np.random.randn(512, 256).astype(np.float32)
    router_W = np.random.randn(256, 8).astype(np.float32) * 0.1
    scores64 = x.astype(np.float64) @ router_W.astype(np.float64)
    route_idx = np.argsort(-scores64, axis=-1)[:, :1].astype(np.int32)
    expert_W = np.random.randn(8, 256, 512).astype(np.float32) * 0.02
    shared_W = np.random.randn(256, 512).astype(np.float32) * 0.02
    return {"x": x, "router_W": router_W, "route_idx": route_idx, "expert_W": expert_W, "shared_W": shared_W}

def reference(x, router_W, route_idx, expert_W, shared_W):
    scores = x @ router_W
    s_max = scores.max(axis=-1, keepdims=True)
    probs = np.exp(scores - s_max)
    probs = probs / probs.sum(axis=-1, keepdims=True)
    shared = x @ shared_W
    out = np.zeros((512, 512), dtype=np.float32)
    for i in range(512):
        e = int(route_idx[i, 0])
        out[i] = shared[i] + probs[i, e] * (x[i] @ expert_W[e])
    return out
```

```python
import functools

import jax
import jax.numpy as jnp
from jax import lax
from jax.experimental import pallas as pl
from jax.experimental.pallas import tpu as pltpu

MESH = pl.DeviceIdType.MESH
BF = jnp.bfloat16
F32 = jnp.float32
I32 = jnp.int32
N_TOK, D, H, N_DEV = 512, 256, 512, 4
BLK = N_TOK // N_DEV
FAST = 64
CLASSES = (32, 40, 48, 64, 128)
ORDER = ((2, 3, 1), (0, 3, 2), (0, 3, 1), (0, 2, 1))


def _dot(a, b):
    return lax.dot_general(a, b, (((1,), (0,)), ((), ())), preferred_element_type=F32)


def _body(x_hbm, rw_hbm, idx_hbm, w_hbm, sw_hbm, o_ref,
          xv, rwv, idxv, wv, swv, ab, sbuf, rbuf, sS, lsem, ssem, rsem):
    me = lax.axis_index("i")
    odd = (me & 1) == 1

    def table(vals):
        r = jnp.int32(vals[3])
        for i in (2, 1, 0):
            r = jnp.where(me == i, vals[i], r)
        return r

    dst = [table([ORDER[i][s] for i in range(N_DEV)]) for s in range(3)]
    blks = dst + [me]
    rslot = [((me - d) & 3) - 1 for d in dst]

    c_idx = pltpu.make_async_copy(idx_hbm, idxv, lsem.at[0])
    c_rw = pltpu.make_async_copy(rw_hbm, rwv, lsem.at[1])
    c_x = [pltpu.make_async_copy(x_hbm.at[pl.ds(blks[s] * BLK, BLK), :], xv.at[s], lsem.at[2 + s])
           for s in range(4)]
    c_w = [pltpu.make_async_copy(w_hbm.at[:, :, pl.ds(n * 128, 128)], wv.at[n], lsem.at[6 + n])
           for n in range(4)]
    c_sw = pltpu.make_async_copy(sw_hbm, swv, lsem.at[10])
    c_idx.start()
    c_x[0].start()
    pl.when(odd)(c_x[1].start)
    for n in range(4):
        c_w[n].start()
    pl.when(jnp.logical_not(odd))(c_x[1].start)
    c_x[2].start()
    c_x[3].start()
    c_rw.start()
    c_sw.start()
    bar = pltpu.get_barrier_semaphore()
    for o in (1, 2, 3):
        pl.semaphore_signal(bar, 1, device_id=((me + o) & 3,), device_id_type=MESH)

    r_io = lax.broadcasted_iota(I32, (BLK, BLK), 0)
    c_io = lax.broadcasted_iota(I32, (BLK, BLK), 1)
    upper = jnp.where(r_io < c_io, 1.0, 0.0).astype(BF)
    c_idx.wait()
    r8 = lax.broadcasted_iota(I32, (8, BLK), 0)
    idx_rows = [idxv[blks[s]] for s in range(4)]
    ids = jnp.zeros((8, BLK), I32)
    tgt = jnp.full((8, BLK), -1, I32)
    for s in range(4):
        ids = jnp.where(r8 == s, idx_rows[s], ids)
        tgt = jnp.where(r8 == s, me, tgt)
    for j in range(3):
        ids = jnp.where(r8 == 4 + j, idx_rows[3], ids)
        tgt = jnp.where(r8 == 4 + j, (me + j + 1) & 3, tgt)
    hit8 = (ids >> 1) == tgt
    pos8 = _dot(jnp.where(hit8, 1.0, 0.0).astype(BF), upper).astype(I32)
    cnt = [jnp.sum(jnp.where(hit8[r:r + 1, :], 1, 0)) for r in range(7)]
    scnt, rcnt = cnt[0:3], cnt[4:7]
    most = cnt[0]
    for c in cnt[1:]:
        most = jnp.maximum(most, c)

    def send_desc(k, n, rows):
        r = pl.ds(0, rows)
        return pltpu.make_async_remote_copy(
            sbuf.at[k, n, r, :], rbuf.at[rslot[k], n, r, :], ssem.at[k, n], rsem.at[rslot[k], n],
            device_id=(dst[k],), device_id_type=MESH)

    def recv_desc(j, n, rows):
        r = pl.ds(0, rows)
        return pltpu.make_async_remote_copy(
            sbuf.at[0, n, r, :], rbuf.at[j, n, r, :], ssem.at[0, n], rsem.at[j, n],
            device_id=(me,), device_id_type=MESH)

    def w_tile(n, kt):
        return wv[n, kt // 2, pl.ds((kt % 2) * 128, 128), :].astype(BF)

    def pipeline(cap, two_first):
        classes = [q for q in CLASSES if q <= cap]

        def by_class(c, fn):
            lo = 0
            for q in classes:
                if lo and q != classes[-1]:
                    cond = (c > lo) & (c <= q)
                elif lo:
                    cond = c > lo
                else:
                    cond = c <= q
                pl.when(cond)(functools.partial(fn, q))
                lo = q

        def send_start(k, n):
            by_class(scnt[k], lambda q: send_desc(k, n, q).start())

        def send_wait(k, n):
            by_class(scnt[k], lambda q: send_desc(k, n, q).wait_send())

        def recv_wait(j, n):
            by_class(rcnt[j], lambda q: recv_desc(j, n, q).wait_recv())

        row = lax.broadcasted_iota(I32, (cap, BLK), 0)
        onehot = []
        for s in range(4):
            at = row == pos8[s:s + 1, :]
            e = idx_rows[s] - 2 * me
            onehot.append(jnp.concatenate(
                [jnp.where(at & (e == 0), 1.0, 0.0).astype(BF),
                 jnp.where(at & (e == 1), 1.0, 0.0).astype(BF)], axis=0))

        def gather(s):
            xc = _dot(onehot[s], xv[s].astype(BF)).astype(BF)
            for e in range(2):
                for h in range(2):
                    ab[s, 2 * e + h, pl.ds(0, cap), :] = xc[e * cap:(e + 1) * cap, h * 128:(h + 1) * 128]

        def expert_chunk(slots, n):
            y = None
            for kt in range(4):
                parts = [ab[s, kt, pl.ds(0, cap), :] for s in slots]
                a = jnp.concatenate(parts, axis=0) if len(parts) > 1 else parts[0]
                t = _dot(a, w_tile(n, kt))
                y = t if y is None else y + t
            return y.astype(BF)

        def serve(slots, n):
            y = expert_chunk(slots, n)
            for i, k in enumerate(slots):
                sbuf[k, n, pl.ds(0, cap), :] = y[i * cap:(i + 1) * cap]

        first = [0, 1] if two_first else [0]
        second = [2] if two_first else [1, 2]
        for s in first:
            c_x[s].wait()
        for s in first:
            gather(s)
        for n in range(4):
            c_w[n].wait()
            serve(first, n)
            if n == 0:
                pl.semaphore_wait(bar, 3)
            for k in first:
                send_start(k, n)
        for s in second:
            c_x[s].wait()
        for s in second:
            gather(s)
        for n in range(4):
            serve(second, n)
            for k in second:
                send_start(k, n)

        c_x[3].wait()
        c_rw.wait()
        c_sw.wait()
        gather(3)
        xb = xv[3].astype(BF)
        scores = lax.dot_general(rwv[...].astype(BF), xb, (((1,), (1,)), ((), ())),
                                 preferred_element_type=F32)
        ex = jnp.exp(scores - jnp.max(scores, axis=0, keepdims=True))
        den = jnp.sum(ex, axis=0, keepdims=True)
        num = jnp.sum(jnp.where(r8 == idx_rows[3], ex, 0.0), axis=0, keepdims=True)
        prob = num / den
        packed = cap <= 64
        koff = [0, 128, 64, 192] if packed else [0, 128, 256, 384]
        slot = koff[3] + pos8[3:4, :]
        for j in range(3):
            slot = jnp.where(hit8[4 + j:5 + j, :], koff[j] + pos8[4 + j:5 + j, :], slot)
        slot_col = jnp.broadcast_to(slot.astype(F32), (BLK, BLK)).T
        prob_col = jnp.broadcast_to(prob, (BLK, BLK)).T
        for j in range(2 if packed else 4):
            sS[j] = jnp.where(slot_col == (c_io + j * 128).astype(F32), prob_col, 0.0).astype(BF)
        for n in range(4):
            rbuf[3, n, pl.ds(0, cap), :] = expert_chunk([3], n)
        for n in range(4):
            o_ref[:, n * 128:(n + 1) * 128] = _dot(xb, swv[:, n * 128:(n + 1) * 128].astype(BF))

        word = lax.broadcasted_iota(I32, (cap // 2, 128), 0)

        def rows_of(j, n):
            r = rbuf[j, n, pl.ds(0, cap), :]
            if j == 3:
                return r
            w = pltpu.bitcast(r, jnp.uint32)
            w = jnp.where(word < ((rcnt[j] + 1) >> 1), w, jnp.uint32(0))
            return pltpu.bitcast(w, BF)

        def scatter(n, terms, parts):
            m = BLK // parts
            for i in range(parts):
                t = None
                for tile, k, r in terms:
                    u = _dot(sS[tile, pl.ds(i * m, m), pl.ds(0, k)], r)
                    t = u if t is None else t + u
                o_ref[pl.ds(i * m, m), n * 128:(n + 1) * 128] += t

        for n in range(4):
            for j in range(3):
                if (j, n) != (1, 3):
                    recv_wait(j, n)
        for n in range(4):
            if packed:
                diag = rows_of(1, n) if n < 3 else jnp.zeros((cap, 128), BF)
                terms = [(0, 128, jnp.concatenate([rows_of(0, n), rows_of(2, n)], axis=0)),
                         (1, 128, jnp.concatenate([diag, rows_of(3, n)], axis=0))]
            else:
                terms = [(j, 128, rows_of(j, n)) for j in range(4) if (j, n) != (1, 3)]
            scatter(n, terms, 2)
        for k in range(3):
            for n in range(4):
                send_wait(k, n)
        recv_wait(1, 3)
        scatter(3, [(1, cap, rows_of(1, 3))], 4)

    fast = most <= FAST
    pl.when(fast & odd)(functools.partial(pipeline, FAST, True))
    pl.when(fast & jnp.logical_not(odd))(functools.partial(pipeline, FAST, False))
    pl.when(jnp.logical_not(fast))(functools.partial(pipeline, BLK, False))


def pallas_dist_moe_shared_ep_outshard_n512_d256_e2_h512_kernel(
    x: jax.Array,
    router_W: jax.Array,
    route_idx: jax.Array,
    expert_W: jax.Array,
    shared_W: jax.Array,
):
    hbm = pl.BlockSpec(memory_space=pl.ANY)
    return pl.pallas_call(
        _body,
        out_shape=jax.ShapeDtypeStruct((BLK, H), F32),
        in_specs=[hbm] * 5,
        out_specs=pl.BlockSpec(memory_space=pltpu.VMEM),
        scratch_shapes=[
            pltpu.VMEM((4, BLK, D), F32),
            pltpu.VMEM((8, D), F32),
            pltpu.VMEM((4, 1, BLK), I32),
            pltpu.VMEM((4, 2, D, 128), F32),
            pltpu.VMEM((D, H), F32),
            pltpu.VMEM((4, 4, BLK, 128), BF),
            pltpu.VMEM((3, 4, BLK, 128), BF),
            pltpu.VMEM((4, 4, BLK, 128), BF),
            pltpu.VMEM((4, BLK, 128), BF),
            pltpu.SemaphoreType.DMA((11,)),
            pltpu.SemaphoreType.DMA((3, 4)),
            pltpu.SemaphoreType.DMA((3, 4)),
        ],
        compiler_params=pltpu.CompilerParams(
            collective_id=0, disable_bounds_checks=True, disable_semaphore_checks=True),
    )(x, router_W.T, route_idx.reshape(4, 1, BLK), expert_W, shared_W)
```

```python
import functools

import jax
import jax.numpy as jnp
from jax import lax
from jax.experimental import pallas as pl
from jax.experimental.pallas import tpu as pltpu

MESH = pl.DeviceIdType.MESH
BF = jnp.bfloat16
F32 = jnp.float32
I32 = jnp.int32
N_TOK, D, H, N_DEV = 512, 256, 512, 4
BLK = N_TOK // N_DEV
FAST = 32
CLASSES = (16, 24, 32, 64, 128)
ORDER = ((2, 3, 1), (0, 3, 2), (0, 3, 1), (0, 2, 1))
SRC = ((1, 2, 3), (0, 2, 3), (3, 0, 1), (0, 2, 1))
SLOT = tuple(tuple(SRC[r].index(s) if s in SRC[r] else 0 for s in range(N_DEV)) for r in range(N_DEV))


def _dot(a, b):
    return lax.dot_general(a, b, (((1,), (0,)), ((), ())), preferred_element_type=F32)


def _body(x_hbm, rw_hbm, idx_hbm, w_hbm, sw_hbm, o_ref,
          xv, rwv, idxv, wv, swv, ab, sbuf, rbuf, sS, lsem, ssem, rsem):
    me = lax.axis_index("i")
    odd = (me & 1) == 1

    def table(vals):
        r = jnp.int32(vals[3])
        for i in (2, 1, 0):
            r = jnp.where(me == i, vals[i], r)
        return r

    dst = [table([ORDER[i][s] for i in range(N_DEV)]) for s in range(3)]
    blks = dst + [me]
    rslot = [table([SLOT[ORDER[i][s]][i] for i in range(N_DEV)]) for s in range(3)]
    src = [table([SRC[i][j] for i in range(N_DEV)]) for j in range(3)] + [me]

    c_idx = pltpu.make_async_copy(idx_hbm, idxv, lsem.at[0])
    c_rw = pltpu.make_async_copy(rw_hbm, rwv, lsem.at[1])
    c_x = [pltpu.make_async_copy(x_hbm.at[pl.ds(blks[s] * BLK, BLK), :], xv.at[s], lsem.at[2 + s])
           for s in range(4)]
    c_w = [pltpu.make_async_copy(w_hbm.at[:, :, pl.ds(n * 128, 128)], wv.at[n], lsem.at[6 + n])
           for n in range(3)]
    c_wl = [pltpu.make_async_copy(w_hbm.at[e, :, pl.ds(384, 128)], wv.at[3, e], lsem.at[9 + e])
            for e in range(2)]
    c_sw = pltpu.make_async_copy(sw_hbm, swv, lsem.at[11])
    c_idx.start()
    c_w[0].start()
    c_x[0].start()
    pl.when(odd)(c_x[1].start)
    c_w[1].start()
    c_w[2].start()
    c_wl[0].start()
    c_wl[1].start()
    pl.when(jnp.logical_not(odd))(c_x[1].start)
    c_x[2].start()
    c_x[3].start()
    c_rw.start()
    c_sw.start()
    bar = pltpu.get_barrier_semaphore()
    for o in (1, 2, 3):
        pl.semaphore_signal(bar, 1, device_id=((me + o) & 3,), device_id_type=MESH)

    r_io = lax.broadcasted_iota(I32, (BLK, BLK), 0)
    c_io = lax.broadcasted_iota(I32, (BLK, BLK), 1)
    upper = jnp.where(r_io < c_io, 1.0, 0.0).astype(BF)
    c_idx.wait()
    r8 = lax.broadcasted_iota(I32, (8, BLK), 0)
    idx_rows = [idxv[blks[s]] for s in range(4)]
    ids = jnp.zeros((8, BLK), I32)
    for s in range(3):
        ids = jnp.where((r8 >> 1) == s, idx_rows[s], ids)
    shit = (ids == 2 * me + (r8 & 1)) & (r8 < 6)
    tgt = jnp.zeros((8, BLK), I32)
    for j in range(4):
        tgt = jnp.where((r8 >> 1) == j, 2 * src[j] + (r8 & 1), tgt)
    rhit = idx_rows[3] == tgt
    myrow = jnp.max(jnp.where(rhit, r8, 0), axis=0, keepdims=True)
    both = jnp.concatenate([jnp.where(shit, 1.0, 0.0), jnp.where(rhit, 1.0, 0.0)], axis=0).astype(BF)
    pos16 = _dot(both, upper)
    spos = pos16[0:8].astype(I32)
    rpos = jnp.sum(jnp.where(rhit, pos16[8:16], 0.0), axis=0, keepdims=True).astype(I32)
    scnt = [[jnp.sum(jnp.where(shit[2 * s + e:2 * s + e + 1, :], 1, 0)) for e in range(2)] for s in range(3)]
    rcnt = [[jnp.sum(jnp.where(rhit[2 * j + e:2 * j + e + 1, :], 1, 0)) for e in range(2)] for j in range(4)]
    most = jnp.int32(0)
    for pair in scnt + rcnt:
        for c in pair:
            most = jnp.maximum(most, c)

    def send_desc(k, n, e, rows):
        r = pl.ds(0, rows)
        return pltpu.make_async_remote_copy(
            sbuf.at[k, n, e, r, :], rbuf.at[rslot[k], n, e, r, :], ssem.at[k, n, e], rsem.at[rslot[k], n, e],
            device_id=(dst[k],), device_id_type=MESH)

    def recv_desc(j, n, e, rows):
        r = pl.ds(0, rows)
        return pltpu.make_async_remote_copy(
            sbuf.at[0, n, e, r, :], rbuf.at[j, n, e, r, :], ssem.at[0, n, e], rsem.at[j, n, e],
            device_id=(me,), device_id_type=MESH)

    def w_tile(n, e, h):
        return wv[n, e, pl.ds(h * 128, 128), :].astype(BF)

    def pipeline(cap, two_first):
        classes = [q for q in CLASSES if q <= cap]
        packed = cap <= 32

        def by_class(c, fn):
            lo = 0
            for q in classes:
                if lo and q != classes[-1]:
                    cond = (c > lo) & (c <= q)
                elif lo:
                    cond = c > lo
                else:
                    cond = c <= q
                pl.when(cond)(functools.partial(fn, q))
                lo = q

        def send_start(k, n, e):
            by_class(scnt[k][e], lambda q: send_desc(k, n, e, q).start())

        def send_wait(k, n, e):
            by_class(scnt[k][e], lambda q: send_desc(k, n, e, q).wait_send())

        def recv_wait(j, n, e):
            by_class(rcnt[j][e], lambda q: recv_desc(j, n, e, q).wait_recv())

        row = lax.broadcasted_iota(I32, (cap, BLK), 0)
        onehot = []
        for s in range(4):
            halves = []
            for e in range(2):
                if s < 3:
                    at = (row == spos[2 * s + e:2 * s + e + 1, :]) & shit[2 * s + e:2 * s + e + 1, :]
                else:
                    at = (row == rpos) & (myrow == 6 + e)
                halves.append(jnp.where(at, 1.0, 0.0).astype(BF))
            onehot.append(jnp.concatenate(halves, axis=0))

        def gather(s):
            xc = _dot(onehot[s], xv[s].astype(BF)).astype(BF)
            for e in range(2):
                for h in range(2):
                    ab[s, e, h, pl.ds(0, cap), :] = xc[e * cap:(e + 1) * cap, h * 128:(h + 1) * 128]

        def expert_chunk(slots, n, e):
            y = None
            for h in range(2):
                parts = [ab[s, e, h, pl.ds(0, cap), :] for s in slots]
                a = jnp.concatenate(parts, axis=0) if len(parts) > 1 else parts[0]
                t = _dot(a, w_tile(n, e, h))
                y = t if y is None else y + t
            return y.astype(BF)

        def serve(slots, n, experts):
            for e in experts:
                y = expert_chunk(slots, n, e)
                for i, k in enumerate(slots):
                    sbuf[k, n, e, pl.ds(0, cap), :] = y[i * cap:(i + 1) * cap]

        def send(slots, n, experts):
            for k in slots:
                for e in experts:
                    send_start(k, n, e)

        first = [0, 1] if two_first else [0]
        second = [2] if two_first else [1, 2]
        for s in first:
            c_x[s].wait()
        for s in first:
            gather(s)
        for n in range(3):
            c_w[n].wait()
            serve(first, n, (0, 1))
            if n == 0:
                pl.semaphore_wait(bar, 3)
            send(first, n, (0, 1))
        for e in range(2):
            c_wl[e].wait()
            serve(first, 3, (e,))
            send(first, 3, (e,))
        for s in second:
            c_x[s].wait()
        for s in second:
            gather(s)
        for n in range(4):
            serve(second, n, (0, 1))
            send(second, n, (0, 1))

        c_x[3].wait()
        c_rw.wait()
        c_sw.wait()
        gather(3)
        xb = xv[3].astype(BF)
        scores = lax.dot_general(rwv[...].astype(BF), xb, (((1,), (1,)), ((), ())),
                                 preferred_element_type=F32)
        ex = jnp.exp(scores - jnp.max(scores, axis=0, keepdims=True))
        den = jnp.sum(ex, axis=0, keepdims=True)
        num = jnp.sum(jnp.where(r8 == idx_rows[3], ex, 0.0), axis=0, keepdims=True)
        prob = num / den
        if packed:
            j_of = myrow >> 1
            base = jnp.where(j_of == 0, 0, jnp.where(j_of == 2, 64, jnp.where(j_of == 1, 128, 192))) + (myrow & 1) * 32
        else:
            base = myrow * 128
        slot_col = jnp.broadcast_to((base + rpos).astype(F32), (BLK, BLK)).T
        prob_col = jnp.broadcast_to(prob, (BLK, BLK)).T
        for j in range(2 if packed else 8):
            sS[j] = jnp.where(slot_col == (c_io + j * 128).astype(F32), prob_col, 0.0).astype(BF)
        for n in range(4):
            for e in range(2):
                rbuf[3, n, e, pl.ds(0, cap), :] = expert_chunk([3], n, e)
        for n in range(4):
            o_ref[:, n * 128:(n + 1) * 128] = _dot(xb, swv[:, n * 128:(n + 1) * 128].astype(BF))

        word = lax.broadcasted_iota(I32, (cap // 2, 128), 0)
        zeros = jnp.zeros((cap, 128), BF)

        def rows_of(j, n, e):
            r = rbuf[j, n, e, pl.ds(0, cap), :]
            if j == 3:
                return r
            w = pltpu.bitcast(r, jnp.uint32)
            w = jnp.where(word < ((rcnt[j][e] + 1) >> 1), w, jnp.uint32(0))
            return pltpu.bitcast(w, BF)

        def scatter(n, terms, parts):
            m = BLK // parts
            for i in range(parts):
                t = None
                for tile, k, r in terms:
                    u = _dot(sS[tile, pl.ds(i * m, m), pl.ds(0, k)], r)
                    t = u if t is None else t + u
                o_ref[pl.ds(i * m, m), n * 128:(n + 1) * 128] += t

        def terms_for(n, with_late):
            if packed:
                late = [rows_of(1, n, 0), rows_of(1, n, 1)] if with_late else [zeros, zeros]
                return [(0, 128, jnp.concatenate([rows_of(0, n, 0), rows_of(0, n, 1), rows_of(2, n, 0), rows_of(2, n, 1)], axis=0)),
                        (1, 128, jnp.concatenate(late + [rows_of(3, n, 0), rows_of(3, n, 1)], axis=0))]
            return [(2 * j + e, 128, rows_of(j, n, e))
                    for j in range(4) for e in range(2) if with_late or j != 1]

        def late_terms(n):
            if packed:
                return [(1, 2 * cap, jnp.concatenate([rows_of(1, n, 0), rows_of(1, n, 1)], axis=0))]
            return [(2 + e, 128, rows_of(1, n, e)) for e in range(2)]

        def wait_sends():
            for k in range(3):
                for n in range(4):
                    for e in range(2):
                        send_wait(k, n, e)

        def wait_rows(slots, chunks):
            for n in chunks:
                for j in slots:
                    for e in range(2):
                        recv_wait(j, n, e)

        if two_first:
            wait_rows((0, 1, 2), (0, 1))
            for n in (0, 1):
                scatter(n, terms_for(n, True), 2)
            wait_sends()
            for n in (2, 3):
                wait_rows((0, 1, 2), (n,))
                scatter(n, terms_for(n, True), 2)
        else:
            wait_rows((0, 2), range(4))
            for n in range(4):
                scatter(n, terms_for(n, False), 2)
            wait_sends()
            wait_rows((1,), (0, 1, 2))
            for n in (0, 1, 2):
                scatter(n, late_terms(n), 4)
            wait_rows((1,), (3,))
            scatter(3, late_terms(3), 4)

    fast = most <= FAST
    pl.when(fast & odd)(functools.partial(pipeline, FAST, True))
    pl.when(fast & jnp.logical_not(odd))(functools.partial(pipeline, FAST, False))
    pl.when(jnp.logical_not(fast))(functools.partial(pipeline, BLK, False))


def pallas_dist_moe_shared_ep_outshard_n512_d256_e2_h512_kernel(
    x: jax.Array,
    router_W: jax.Array,
    route_idx: jax.Array,
    expert_W: jax.Array,
    shared_W: jax.Array,
):
    hbm = pl.BlockSpec(memory_space=pl.ANY)
    return pl.pallas_call(
        _body,
        out_shape=jax.ShapeDtypeStruct((BLK, H), F32),
        in_specs=[hbm] * 5,
        out_specs=pl.BlockSpec(memory_space=pltpu.VMEM),
        scratch_shapes=[
            pltpu.VMEM((4, BLK, D), F32),
            pltpu.VMEM((8, D), F32),
            pltpu.VMEM((4, 1, BLK), I32),
            pltpu.VMEM((4, 2, D, 128), F32),
            pltpu.VMEM((D, H), F32),
            pltpu.VMEM((4, 2, 2, BLK, 128), BF),
            pltpu.VMEM((3, 4, 2, BLK, 128), BF),
            pltpu.VMEM((4, 4, 2, BLK, 128), BF),
            pltpu.VMEM((8, BLK, 128), BF),
            pltpu.SemaphoreType.DMA((12,)),
            pltpu.SemaphoreType.DMA((3, 4, 2)),
            pltpu.SemaphoreType.DMA((3, 4, 2)),
        ],
        compiler_params=pltpu.CompilerParams(
            collective_id=0, disable_bounds_checks=True, disable_semaphore_checks=True),
    )(x, router_W.T, route_idx.reshape(4, 1, BLK), expert_W, shared_W)
```
